```python
import numpy as np

kernel_name = "dist_layernorm_xy_m6144_n2048"

def setup_inputs():
    x = np.random.randn(12288, 4096).astype(np.float32)
    gamma = np.random.randn(4096).astype(np.float32)
    beta = np.random.randn(4096).astype(np.float32)
    return {"x": x, "gamma": gamma, "beta": beta}

def reference(x: np.ndarray, gamma: np.ndarray, beta: np.ndarray) -> np.ndarray:
    eps = 1e-5
    mean = np.mean(x, axis=1, keepdims=True)
    var = np.var(x, axis=1, keepdims=True)
    return gamma * (x - mean) / np.sqrt(var + eps) + beta
```

```python
import jax
import jax.numpy as jnp
from jax import lax
from jax.experimental import pallas as pl
from jax.experimental.pallas import tpu as pltpu

EPS = 1e-5
OUT_DTYPE = jnp.bfloat16

LANES = 128
SUB = 8
BLOCK = 192
TAIL = (96, 64, 32)
WINDOW = 3
N_RSEM = 4
TILE = 32


def _tree_sum(vals):
    vals = list(vals)
    while len(vals) > 1:
        vals = [
            vals[i] + vals[i + 1] if i + 1 < len(vals) else vals[i]
            for i in range(0, len(vals), 2)
        ]
    return vals[0]


def pallas_dist_layernorm_xy_m6144_n2048_kernel(
    x: jax.Array,
    gamma: jax.Array,
    beta: jax.Array,
):
    m, n = x.shape
    n_chunks = n // LANES
    n_main = (m - sum(TAIL)) // BLOCK
    assert n_main * BLOCK + sum(TAIL) == m and n_main > WINDOW
    assert n % LANES == 0 and BLOCK // SUB <= LANES and max(TAIL) <= BLOCK
    sizes = [BLOCK] * n_main + list(TAIL)
    starts = [sum(sizes[:i]) for i in range(len(sizes))]
    n_blocks = len(sizes)
    n_total = 2 * n

    def body(x_hbm, g_hbm, b_hbm, o_ref,
             xbuf, gb_raw, gb, mu_buf, m2_buf, mr_buf, st_own, st_nbr,
             read_sems, gb_sem, send_sem, recv_sems):
        nbr = (lax.axis_index("x"), 1 - lax.axis_index("y"))

        def read(i):
            if isinstance(i, int):
                start, size = starts[i], sizes[i]
                sem = read_sems.at[i % N_RSEM if i < n_main else N_RSEM + i - n_main]
            else:
                start, size = pl.multiple_of(i * BLOCK, TILE), BLOCK
                sem = read_sems.at[lax.rem(i, N_RSEM)]
            rows = pl.ds(start, size)
            return pltpu.make_async_copy(x_hbm.at[rows], xbuf.at[rows], sem)

        def exchange(i):
            return pltpu.make_async_remote_copy(
                src_ref=st_own.at[i], dst_ref=st_nbr.at[i],
                send_sem=send_sem, recv_sem=recv_sems.at[i],
                device_id=nbr, device_id_type=pl.DeviceIdType.MESH)

        lane = lax.broadcasted_iota(jnp.int32, (SUB, LANES), 1)

        def row_loop(size, step):
            if size == TILE:
                step(0)
            else:
                def it(t, carry):
                    step(pl.multiple_of(t * TILE, TILE))
                    return carry
                lax.fori_loop(0, size // TILE, it, 0)

        def stats(i, start, size):
            def step(t0):
                rows = pl.ds(pl.multiple_of(start + t0, TILE), TILE)
                xs = [xbuf[rows, c * LANES:(c + 1) * LANES] for c in range(n_chunks)]
                mu = _tree_sum(xs) * (1.0 / n_chunks)
                m2 = _tree_sum([(v - mu) * (v - mu) for v in xs])
                mu_buf[pl.ds(t0, TILE), :] = mu
                m2_buf[pl.ds(t0, TILE), :] = m2
            row_loop(size, step)
            mu = mu_buf[0:size, :]
            mean = jnp.sum(mu, axis=1, keepdims=True) * (1.0 / LANES)
            dev = mu - mean
            m2 = jnp.sum(m2_buf[0:size, :] + (float(n_chunks) * dev) * dev, axis=1, keepdims=True)
            p_mean = jnp.zeros((SUB, LANES), jnp.float32)
            p_m2 = jnp.zeros((SUB, LANES), jnp.float32)
            for j in range(size // SUB):
                p_mean = jnp.where(lane == j, mean[SUB * j:SUB * (j + 1)], p_mean)
                p_m2 = jnp.where(lane == j, m2[SUB * j:SUB * (j + 1)], p_m2)
            st_own[i, 0:SUB, :] = p_mean
            st_own[i, SUB:2 * SUB, :] = p_m2

        def normalise(i, start, size):
            mean_a, m2_a = st_own[i, 0:SUB, :], st_own[i, SUB:2 * SUB, :]
            mean_b, m2_b = st_nbr[i, 0:SUB, :], st_nbr[i, SUB:2 * SUB, :]
            mean = (mean_a + mean_b) * 0.5
            delta = mean_a - mean_b
            var = (m2_a + m2_b + delta * delta * (n / 2.0)) * (1.0 / n_total)
            rstd = lax.rsqrt(var + EPS)
            for j in range(size // SUB):
                for k, v in enumerate((mean, rstd)):
                    col = jnp.sum(jnp.where(lane == j, v, 0.0), axis=1, keepdims=True)
                    mr_buf[k, SUB * j:SUB * (j + 1), :] = jnp.broadcast_to(col, (SUB, LANES))

            def step(t0):
                rows = pl.ds(pl.multiple_of(start + t0, TILE), TILE)
                row_mean = mr_buf[0, pl.ds(t0, TILE), :]
                row_rstd = mr_buf[1, pl.ds(t0, TILE), :]
                for c in range(n_chunks):
                    cols = slice(c * LANES, (c + 1) * LANES)
                    g = jnp.concatenate([gb[0:SUB, cols]] * (TILE // SUB), axis=0)
                    b = jnp.concatenate([gb[SUB:2 * SUB, cols]] * (TILE // SUB), axis=0)
                    y = (xbuf[rows, cols] - row_mean) * row_rstd * g + b
                    o_ref[rows, cols] = y.astype(o_ref.dtype)
            row_loop(size, step)

        read(0).start()
        barrier = pltpu.get_barrier_semaphore()
        pl.semaphore_signal(barrier, inc=1, device_id=nbr, device_id_type=pl.DeviceIdType.MESH)
        for i in range(1, WINDOW):
            read(i).start()
        pltpu.make_async_copy(g_hbm, gb_raw.at[pl.ds(0, 1)], gb_sem).start()
        pltpu.make_async_copy(b_hbm, gb_raw.at[pl.ds(1, 1)], gb_sem).start()

        def main_step(i, carry):
            read(i).wait()

            @pl.when(i + WINDOW < n_main)
            def _():
                read(i + WINDOW).start()

            @pl.when(i + WINDOW == n_main)
            def _():
                for j in range(n_main, n_blocks):
                    read(j).start()

            stats(i, pl.multiple_of(i * BLOCK, TILE), BLOCK)

            @pl.when(i == 0)
            def _():
                pl.semaphore_wait(barrier, 1)

            exchange(i).start()

            @pl.when(i == 0)
            def _():
                pltpu.make_async_copy(gb_raw, gb_raw, gb_sem).wait()
                gb[0:SUB, :] = jnp.broadcast_to(gb_raw[0:1, :], (SUB, n))
                gb[SUB:2 * SUB, :] = jnp.broadcast_to(gb_raw[1:2, :], (SUB, n))

            @pl.when(i >= 1)
            def _():
                exchange(i - 1).wait_recv()
                normalise(i - 1, pl.multiple_of((i - 1) * BLOCK, TILE), BLOCK)

            return carry

        lax.fori_loop(0, n_main, main_step, 0)

        def finish(j):
            exchange(j).wait_recv()
            normalise(j, starts[j], sizes[j])

        for j in range(n_main, n_blocks):
            read(j).wait()
            stats(j, starts[j], sizes[j])
            exchange(j).start()
            if j == n_main:
                finish(n_main - 1)
        for j in range(n_main, n_blocks):
            finish(j)
        pltpu.make_async_copy(st_own, st_own, send_sem).wait()

    f32 = jnp.float32
    return pl.pallas_call(
        body,
        out_shape=pltpu.VMEM((m, n), OUT_DTYPE),
        in_specs=[pl.BlockSpec(memory_space=pl.ANY)] * 3,
        out_specs=pl.BlockSpec(memory_space=pltpu.VMEM),
        scratch_shapes=[
            pltpu.VMEM((m, n), f32),
            pltpu.VMEM((2, n), f32),
            pltpu.VMEM((2 * SUB, n), f32),
            pltpu.VMEM((BLOCK, LANES), f32),
            pltpu.VMEM((BLOCK, LANES), f32),
            pltpu.VMEM((2, BLOCK, LANES), f32),
            pltpu.VMEM((n_blocks, 2 * SUB, LANES), f32),
            pltpu.VMEM((n_blocks, 2 * SUB, LANES), f32),
            pltpu.SemaphoreType.DMA((N_RSEM + len(TAIL),)),
            pltpu.SemaphoreType.DMA,
            pltpu.SemaphoreType.DMA,
            pltpu.SemaphoreType.DMA((n_blocks,)),
        ],
        compiler_params=pltpu.CompilerParams(
            collective_id=0, vmem_limit_bytes=64 * 2**20),
    )(x, gamma.reshape(1, n), beta.reshape(1, n))
```

```python
import jax
import jax.numpy as jnp
from jax import lax
from jax.experimental import pallas as pl
from jax.experimental.pallas import tpu as pltpu

EPS = 1e-5
OUT_DTYPE = jnp.bfloat16

LANES = 128
SUB = 8
TILE = 32
BLOCK = 768
TAIL = (256, 192, 128, 96, 64, 32)
WINDOW = 2


def _tree_sum(vals):
    vals = list(vals)
    while len(vals) > 1:
        vals = [
            vals[i] + vals[i + 1] if i + 1 < len(vals) else vals[i]
            for i in range(0, len(vals), 2)
        ]
    return vals[0]


def _slots(rows):
    return -(-rows // LANES)


def pallas_dist_layernorm_xy_m6144_n2048_kernel(
    x: jax.Array,
    gamma: jax.Array,
    beta: jax.Array,
):
    m, n = x.shape
    n_chunks = n // LANES
    n_main = (m - sum(TAIL)) // BLOCK
    sizes = [BLOCK] * n_main + list(TAIL)
    n_blocks = len(sizes)
    assert n % LANES == 0 and sum(sizes) == m and n_main >= WINDOW
    assert all(s % TILE == 0 and s <= BLOCK for s in sizes)
    starts = [sum(sizes[:i]) for i in range(n_blocks)]
    first_slot = [sum(_slots(s) for s in sizes[:i]) for i in range(n_blocks)]
    n_slots = sum(_slots(s) for s in sizes)
    n_row = 2 * n

    def body(x_hbm, g_hbm, b_hbm, o_ref,
             xbuf, gb_raw, gb, mu_buf, m2_buf, mr_buf, st_own, st_nbr,
             read_sems, gb_sem, send_sem, recv_sems):
        def geometry(i):
            if isinstance(i, int):
                return starts[i], sizes[i], first_slot[i]
            return pl.multiple_of(i * BLOCK, TILE), BLOCK, i * _slots(BLOCK)

        def read(i):
            start, size, _ = geometry(i)
            if isinstance(i, int):
                sem = read_sems.at[i % WINDOW if i < n_main else WINDOW + i - n_main]
            else:
                sem = read_sems.at[lax.rem(i, WINDOW)]
            rows = pl.ds(start, size)
            return pltpu.make_async_copy(x_hbm.at[rows], xbuf.at[rows], sem)

        read(0).start()

        nbr = (lax.axis_index("x"), 1 - lax.axis_index("y"))

        def exchange(i):
            _, size, slot = geometry(i)
            slots = pl.ds(slot, _slots(size))
            return pltpu.make_async_remote_copy(
                src_ref=st_own.at[slots], dst_ref=st_nbr.at[slots],
                send_sem=send_sem, recv_sem=recv_sems.at[i],
                device_id=nbr, device_id_type=pl.DeviceIdType.MESH)

        diag = (lax.broadcasted_iota(jnp.int32, (SUB, LANES), 1)
                - lax.broadcasted_iota(jnp.int32, (SUB, LANES), 0))

        def row_loop(size, step):
            if size == TILE:
                step(0)
            else:
                def it(t, carry):
                    step(pl.multiple_of(t * TILE, TILE))
                    return carry
                lax.fori_loop(0, size // TILE, it, 0)

        def stats(i):
            start, size, slot = geometry(i)

            def step(t0):
                rows = pl.ds(pl.multiple_of(start + t0, TILE), TILE)
                xs = [xbuf[rows, c * LANES:(c + 1) * LANES] for c in range(n_chunks)]
                mu = _tree_sum(xs) * (1.0 / n_chunks)
                m2 = _tree_sum([(v - mu) * (v - mu) for v in xs])
                mu_buf[pl.ds(t0, TILE), :] = mu
                m2_buf[pl.ds(t0, TILE), :] = m2

            row_loop(size, step)
            mu = mu_buf[0:size, :]
            mean = jnp.sum(mu, axis=1, keepdims=True) * (1.0 / LANES)
            dev = mu - mean
            m2 = jnp.sum(m2_buf[0:size, :] + (float(n_chunks) * dev) * dev,
                         axis=1, keepdims=True)
            for q in range(_slots(size)):
                p_mean = jnp.zeros((SUB, LANES), jnp.float32)
                p_m2 = jnp.zeros((SUB, LANES), jnp.float32)
                for r in range(q * LANES, min((q + 1) * LANES, size), SUB):
                    hit = diag == r - q * LANES
                    p_mean = jnp.where(hit, mean[r:r + SUB], p_mean)
                    p_m2 = jnp.where(hit, m2[r:r + SUB], p_m2)
                st_own[slot + q, 0:1, :] = jnp.sum(p_mean, axis=0, keepdims=True)
                st_own[slot + q, 1:2, :] = jnp.sum(p_m2, axis=0, keepdims=True)

        def normalise(i):
            start, size, slot = geometry(i)
            for q in range(_slots(size)):
                mean_a, m2_a = st_own[slot + q, 0:1, :], st_own[slot + q, 1:2, :]
                mean_b, m2_b = st_nbr[slot + q, 0:1, :], st_nbr[slot + q, 1:2, :]
                mean = (mean_a + mean_b) * 0.5
                delta = mean_a - mean_b
                var = (m2_a + m2_b + delta * delta * (n / 2.0)) * (1.0 / n_row)
                rstd = lax.rsqrt(var + EPS)
                for k, v in enumerate((mean, rstd)):
                    v = jnp.broadcast_to(v, (SUB, LANES))
                    for r in range(q * LANES, min((q + 1) * LANES, size), SUB):
                        picked = jnp.where(diag == r - q * LANES, v, 0.0)
                        col = jnp.sum(picked, axis=1, keepdims=True)
                        mr_buf[k, r:r + SUB, :] = jnp.broadcast_to(col, (SUB, LANES))

            def step(t0):
                rows = pl.ds(pl.multiple_of(start + t0, TILE), TILE)
                row_mean = mr_buf[0, pl.ds(t0, TILE), :]
                row_rstd = mr_buf[1, pl.ds(t0, TILE), :]
                for c in range(n_chunks):
                    cols = slice(c * LANES, (c + 1) * LANES)
                    g = jnp.concatenate([gb[0:SUB, cols]] * (TILE // SUB), axis=0)
                    b = jnp.concatenate([gb[SUB:2 * SUB, cols]] * (TILE // SUB), axis=0)
                    y = (xbuf[rows, cols] - row_mean) * row_rstd * g + b
                    o_ref[rows, cols] = y.astype(o_ref.dtype)

            row_loop(size, step)

        def finish(i):
            exchange(i).wait_recv()
            normalise(i)

        barrier = pltpu.get_barrier_semaphore()
        pl.semaphore_signal(barrier, inc=1, device_id=nbr,
                            device_id_type=pl.DeviceIdType.MESH)
        for i in range(1, WINDOW):
            read(i).start()
        pltpu.make_async_copy(g_hbm, gb_raw.at[pl.ds(0, 1)], gb_sem).start()
        pltpu.make_async_copy(b_hbm, gb_raw.at[pl.ds(1, 1)], gb_sem).start()

        def main_step(i, carry):
            read(i).wait()

            @pl.when(i + WINDOW < n_main)
            def _():
                read(jnp.minimum(i + WINDOW, n_main - 1)).start()

            @pl.when(i + WINDOW == n_main)
            def _():
                for j in range(n_main, n_blocks):
                    read(j).start()

            stats(i)

            @pl.when(i == 0)
            def _():
                pl.semaphore_wait(barrier, 1)

            exchange(i).start()

            @pl.when(i == 0)
            def _():
                pltpu.make_async_copy(gb_raw, gb_raw, gb_sem).wait()
                gb[0:SUB, :] = jnp.broadcast_to(gb_raw[0:1, :], (SUB, n))
                gb[SUB:2 * SUB, :] = jnp.broadcast_to(gb_raw[1:2, :], (SUB, n))

            @pl.when(i >= 1)
            def _():
                finish(jnp.maximum(i - 1, 0))

            return carry

        lax.fori_loop(0, n_main, main_step, 0)

        for j in range(n_main, n_blocks):
            read(j).wait()
            stats(j)
            exchange(j).start()
            if j == n_main:
                finish(n_main - 1)
        for j in range(n_main, n_blocks):
            finish(j)
        pltpu.make_async_copy(st_own, st_own, send_sem).wait()

    f32 = jnp.float32
    return pl.pallas_call(
        body,
        out_shape=pltpu.VMEM((m, n), OUT_DTYPE),
        in_specs=[pl.BlockSpec(memory_space=pl.ANY)] * 3,
        out_specs=pl.BlockSpec(memory_space=pltpu.VMEM),
        scratch_shapes=[
            pltpu.VMEM((m, n), f32),
            pltpu.VMEM((2, n), f32),
            pltpu.VMEM((2 * SUB, n), f32),
            pltpu.VMEM((BLOCK, LANES), f32),
            pltpu.VMEM((BLOCK, LANES), f32),
            pltpu.VMEM((2, BLOCK, LANES), f32),
            pltpu.VMEM((n_slots, 2, LANES), f32),
            pltpu.VMEM((n_slots, 2, LANES), f32),
            pltpu.SemaphoreType.DMA((WINDOW + len(TAIL),)),
            pltpu.SemaphoreType.DMA,
            pltpu.SemaphoreType.DMA,
            pltpu.SemaphoreType.DMA((n_blocks,)),
        ],
        compiler_params=pltpu.CompilerParams(
            collective_id=0, vmem_limit_bytes=64 * 2**20),
    )(x, gamma.reshape(1, n), beta.reshape(1, n))
```

```python
import jax
import jax.numpy as jnp
from jax import lax
from jax.experimental import pallas as pl
from jax.experimental.pallas import tpu as pltpu

EPS = 1e-5
OUT_DTYPE = jnp.bfloat16

LANES = 128
SUB = 8
TILE = 32
BLOCK = 768
TAIL = (256, 192, 128, 96, 64, 32)
WINDOW = 2


def _tree_sum(vals):
    vals = list(vals)
    while len(vals) > 1:
        vals = [
            vals[i] + vals[i + 1] if i + 1 < len(vals) else vals[i]
            for i in range(0, len(vals), 2)
        ]
    return vals[0]


def _slots(rows):
    return -(-rows // LANES)


def pallas_dist_layernorm_xy_m6144_n2048_kernel(
    x: jax.Array,
    gamma: jax.Array,
    beta: jax.Array,
):
    m, n = x.shape
    n_chunks = n // LANES
    n_main = (m - sum(TAIL)) // BLOCK
    sizes = [BLOCK] * n_main + list(TAIL)
    n_blocks = len(sizes)
    assert n % LANES == 0 and sum(sizes) == m and n_main >= WINDOW
    assert all(s % TILE == 0 and s <= BLOCK for s in sizes)
    starts = [sum(sizes[:i]) for i in range(n_blocks)]
    first_slot = [sum(_slots(s) for s in sizes[:i]) for i in range(n_blocks)]
    n_slots = sum(_slots(s) for s in sizes)
    n_row = 2 * n

    def body(x_hbm, g_hbm, b_hbm, o_ref,
             xbuf, gb_raw, gb, mu_buf, m2_buf, mr_buf, st_own, st_nbr,
             send_sem, recv_sems):
        def geometry(i):
            if isinstance(i, int):
                return starts[i], sizes[i], first_slot[i]
            return pl.multiple_of(i * BLOCK, TILE), BLOCK, i * _slots(BLOCK)

        def read(i, read_sems):
            start, size, _ = geometry(i)
            if isinstance(i, int):
                sem = read_sems.at[i % WINDOW if i < n_main else WINDOW + i - n_main]
            else:
                sem = read_sems.at[lax.rem(i, WINDOW)]
            rows = pl.ds(start, size)
            return pltpu.make_async_copy(x_hbm.at[rows], xbuf.at[rows], sem)

        nbr = (lax.axis_index("x"), 1 - lax.axis_index("y"))

        def exchange(i):
            _, size, slot = geometry(i)
            slots = pl.ds(slot, _slots(size))
            return pltpu.make_async_remote_copy(
                src_ref=st_own.at[slots], dst_ref=st_nbr.at[slots],
                send_sem=send_sem, recv_sem=recv_sems.at[i],
                device_id=nbr, device_id_type=pl.DeviceIdType.MESH)

        diag = (lax.broadcasted_iota(jnp.int32, (SUB, LANES), 1)
                - lax.broadcasted_iota(jnp.int32, (SUB, LANES), 0))

        def row_loop(size, step):
            if size == TILE:
                step(0)
            else:
                def it(t, carry):
                    step(pl.multiple_of(t * TILE, TILE))
                    return carry
                lax.fori_loop(0, size // TILE, it, 0)

        def stats(i):
            start, size, slot = geometry(i)

            def step(t0):
                rows = pl.ds(pl.multiple_of(start + t0, TILE), TILE)
                xs = [xbuf[rows, c * LANES:(c + 1) * LANES] for c in range(n_chunks)]
                mu = _tree_sum(xs) * (1.0 / n_chunks)
                m2 = _tree_sum([(v - mu) * (v - mu) for v in xs])
                mu_buf[pl.ds(t0, TILE), :] = mu
                m2_buf[pl.ds(t0, TILE), :] = m2

            row_loop(size, step)
            mu = mu_buf[0:size, :]
            mean = jnp.sum(mu, axis=1, keepdims=True) * (1.0 / LANES)
            dev = mu - mean
            m2 = jnp.sum(m2_buf[0:size, :] + (float(n_chunks) * dev) * dev,
                         axis=1, keepdims=True)
            for q in range(_slots(size)):
                p_mean = jnp.zeros((SUB, LANES), jnp.float32)
                p_m2 = jnp.zeros((SUB, LANES), jnp.float32)
                for r in range(q * LANES, min((q + 1) * LANES, size), SUB):
                    hit = diag == r - q * LANES
                    p_mean = jnp.where(hit, mean[r:r + SUB], p_mean)
                    p_m2 = jnp.where(hit, m2[r:r + SUB], p_m2)
                st_own[slot + q, 0:1, :] = jnp.sum(p_mean, axis=0, keepdims=True)
                st_own[slot + q, 1:2, :] = jnp.sum(p_m2, axis=0, keepdims=True)

        def normalise(i):
            start, size, slot = geometry(i)
            for q in range(_slots(size)):
                mean_a, m2_a = st_own[slot + q, 0:1, :], st_own[slot + q, 1:2, :]
                mean_b, m2_b = st_nbr[slot + q, 0:1, :], st_nbr[slot + q, 1:2, :]
                mean = (mean_a + mean_b) * 0.5
                delta = mean_a - mean_b
                var = (m2_a + m2_b + delta * delta * (n / 2.0)) * (1.0 / n_row)
                rstd = lax.rsqrt(var + EPS)
                for k, v in enumerate((mean, rstd)):
                    v = jnp.broadcast_to(v, (SUB, LANES))
                    for r in range(q * LANES, min((q + 1) * LANES, size), SUB):
                        picked = jnp.where(diag == r - q * LANES, v, 0.0)
                        col = jnp.sum(picked, axis=1, keepdims=True)
                        mr_buf[k, r:r + SUB, :] = jnp.broadcast_to(col, (SUB, LANES))

            def step(t0):
                rows = pl.ds(pl.multiple_of(start + t0, TILE), TILE)
                row_mean = mr_buf[0, pl.ds(t0, TILE), :]
                row_rstd = mr_buf[1, pl.ds(t0, TILE), :]
                for c in range(n_chunks):
                    cols = slice(c * LANES, (c + 1) * LANES)
                    g = jnp.concatenate([gb[0:SUB, cols]] * (TILE // SUB), axis=0)
                    b = jnp.concatenate([gb[SUB:2 * SUB, cols]] * (TILE // SUB), axis=0)
                    y = (xbuf[rows, cols] - row_mean) * row_rstd * g + b
                    o_ref[rows, cols] = y.astype(o_ref.dtype)

            row_loop(size, step)

        def finish(i):
            exchange(i).wait_recv()
            normalise(i)

        def stream(read_sems, gb_sem):
            read(0, read_sems).start()
            barrier = pltpu.get_barrier_semaphore()
            pl.semaphore_signal(barrier, inc=1, device_id=nbr,
                                device_id_type=pl.DeviceIdType.MESH)
            for i in range(1, WINDOW):
                read(i, read_sems).start()
            pltpu.make_async_copy(g_hbm, gb_raw.at[pl.ds(0, 1)], gb_sem).start()
            pltpu.make_async_copy(b_hbm, gb_raw.at[pl.ds(1, 1)], gb_sem).start()

            def main_step(i, carry):
                read(i, read_sems).wait()

                @pl.when(i + WINDOW < n_main)
                def _():
                    read(jnp.minimum(i + WINDOW, n_main - 1), read_sems).start()

                @pl.when(i + WINDOW == n_main)
                def _():
                    for j in range(n_main, n_blocks):
                        read(j, read_sems).start()

                stats(i)

                @pl.when(i == 0)
                def _():
                    pl.semaphore_wait(barrier, 1)

                exchange(i).start()

                @pl.when(i == 0)
                def _():
                    pltpu.make_async_copy(gb_raw, gb_raw, gb_sem).wait()
                    gb[0:SUB, :] = jnp.broadcast_to(gb_raw[0:1, :], (SUB, n))
                    gb[SUB:2 * SUB, :] = jnp.broadcast_to(gb_raw[1:2, :], (SUB, n))

                @pl.when(i >= 1)
                def _():
                    finish(jnp.maximum(i - 1, 0))

                return carry

            lax.fori_loop(0, n_main, main_step, 0)

            for j in range(n_main, n_blocks):
                read(j, read_sems).wait()
                stats(j)
                exchange(j).start()
                if j == n_main:
                    finish(n_main - 1)

        pl.run_scoped(stream,
                      pltpu.SemaphoreType.DMA((WINDOW + len(TAIL),)),
                      pltpu.SemaphoreType.DMA)
        for j in range(n_main, n_blocks):
            finish(j)
        pltpu.make_async_copy(st_own, st_own, send_sem).wait()

    f32 = jnp.float32
    return pl.pallas_call(
        body,
        out_shape=pltpu.VMEM((m, n), OUT_DTYPE),
        in_specs=[pl.BlockSpec(memory_space=pl.ANY)] * 3,
        out_specs=pl.BlockSpec(memory_space=pltpu.VMEM),
        scratch_shapes=[
            pltpu.VMEM((m, n), f32),
            pltpu.VMEM((2, n), f32),
            pltpu.VMEM((2 * SUB, n), f32),
            pltpu.VMEM((BLOCK, LANES), f32),
            pltpu.VMEM((BLOCK, LANES), f32),
            pltpu.VMEM((2, BLOCK, LANES), f32),
            pltpu.VMEM((n_slots, 2, LANES), f32),
            pltpu.VMEM((n_slots, 2, LANES), f32),
            pltpu.SemaphoreType.DMA,
            pltpu.SemaphoreType.DMA((n_blocks,)),
        ],
        compiler_params=pltpu.CompilerParams(
            collective_id=0, vmem_limit_bytes=64 * 2**20),
    )(x, gamma.reshape(1, n), beta.reshape(1, n))
```
